```python
import numpy as np

kernel_name = "dist_mean_ax1_xy_m4096_n1024"

def setup_inputs():
    return {"x": np.random.randn(8192, 2048).astype(np.float32)}

def reference(x: np.ndarray) -> np.ndarray:
    return np.mean(x, axis=1, keepdims=True)
```

```python
import jax
import jax.numpy as jnp
from jax import lax
from jax.experimental import pallas as pl
from jax.experimental.pallas import tpu as pltpu

MESH = pl.DeviceIdType.MESH

def make(shift=7, ahead=12, scopes=False):
    NS = 8
    SEG = 32
    NR = 2 * SEG
    STREAM_ORDER = [0, 4, 2, 6, 1, 5, 3, 7]

    def kern(x):
        m, n = x.shape
        scale = 1.0 / (2 * n)

        def body(x_ref, o_ref, buf, part, recv, ld_sem, send_sem, recv_sem):
            mx = lax.axis_index("x")
            my = lax.axis_index("y")
            peer = (mx, 1 - my)

            def seg_tile0(phase):
                half = jnp.where(phase == 0, 1 - my, my)
                return half * (SEG * 8)

            def issue(t0, size, sem):
                for k, s in enumerate(STREAM_ORDER):
                    sl = pl.ds(s * 512 + t0, size)
                    pltpu.make_async_copy(x_ref.at[sl], buf.at[sl], sem).start(priority=k % 2)

            def start_round(r):
                phase = r // SEG
                g = r % SEG
                base = seg_tile0(phase)
                sem = ld_sem.at[r]
                if shift == 0:
                    issue(base + g * 8, 8, sem)
                else:
                    @pl.when(g == 0)
                    def _():
                        issue(base, shift, sem)
                    @pl.when(g < SEG - 1)
                    def _():
                        issue(base + g * 8 + shift, 8, sem)
                    @pl.when(g == SEG - 1)
                    def _():
                        issue(base + g * 8 + shift, 8 - shift, sem)

            def wait_tiles(nt, sem):
                d = buf.at[pl.ds(0, nt)]
                pltpu.make_async_copy(d, d, sem).wait()

            def wait_round(r):
                g = r % SEG
                sem = ld_sem.at[r]
                if shift == 0:
                    wait_tiles(NS * 8, sem)
                else:
                    @pl.when(g == 0)
                    def _():
                        wait_tiles(NS * (8 + shift), sem)
                    @pl.when(jnp.logical_and(g > 0, g < SEG - 1))
                    def _():
                        wait_tiles(NS * 8, sem)
                    @pl.when(g == SEG - 1)
                    def _():
                        wait_tiles(NS * (8 - shift), sem)

            lax.fori_loop(0, ahead, lambda r, _: start_round(r), None)

            bar = pltpu.get_barrier_semaphore()
            pl.semaphore_signal(bar, inc=1, device_id=peer, device_id_type=MESH)

            diag = lax.broadcasted_iota(jnp.int32, (8, 128), 1) - lax.broadcasted_iota(jnp.int32, (8, 128), 0)
            sub = lax.broadcasted_iota(jnp.int32, (8, 128), 0)

            def round_body(r, accs):
                wait_round(r)
                @pl.when(r + ahead < NR)
                def _():
                    start_round(r + ahead)
                t0 = seg_tile0(r // SEG) + (r % SEG) * 8
                mask = diag == (r % 16) * 8
                out = []
                for s in range(NS):
                    v = buf[pl.ds(s * 512 + t0, 8)]
                    p = ((v[0] + v[1]) + (v[2] + v[3])) + ((v[4] + v[5]) + (v[6] + v[7]))
                    rs = jnp.sum(p, axis=1, keepdims=True)
                    out.append(jnp.where(mask, rs, accs[s]))
                return tuple(out)

            def block(b):
                z = jnp.zeros((8, 128), jnp.float32)
                accs = lax.fori_loop(b * 16, b * 16 + 16, round_body, (z,) * NS)
                res = z
                for s in range(NS):
                    res = jnp.where(sub == s, jnp.sum(accs[s], axis=0, keepdims=True), res)
                return res

            def rdma(src, dst, i):
                return pltpu.make_async_remote_copy(src, dst, send_sem.at[i], recv_sem.at[i], device_id=peer, device_id_type=MESH)

            for b in range(2):
                part[b] = block(b)
            pl.semaphore_wait(bar, 1)
            c0 = rdma(part, recv, 0)
            c0.start()
            cs = []
            for b in range(2):
                res = block(2 + b)
                if b == 0:
                    c0.wait_recv()
                j = my * 2 + b
                o_ref[:, pl.ds(j, 1), :] = ((res + recv[b]) * scale)[:, None, :]
                d = o_ref.at[:, pl.ds(j, 1)]
                c = rdma(d, d, 1 + b)
                c.start()
                cs.append(c)
            c0.wait_send()
            for c in cs:
                c.wait()

        xt = x.reshape(m // 8, 8, n // 128, 128).transpose(0, 2, 1, 3).reshape(m * n // 1024, 8, 128)
        o = pl.pallas_call(
            body,
            out_shape=jax.ShapeDtypeStruct((8, 4, 128), jnp.float32),
            in_specs=[pl.BlockSpec(memory_space=pl.ANY)],
            out_specs=pl.BlockSpec(memory_space=pltpu.VMEM),
            scratch_shapes=[
                pltpu.VMEM(xt.shape, jnp.float32),
                pltpu.VMEM((2, 8, 128), jnp.float32),
                pltpu.VMEM((2, 8, 128), jnp.float32),
                pltpu.SemaphoreType.DMA((NR,)),
                pltpu.SemaphoreType.DMA((3,)),
                pltpu.SemaphoreType.DMA((3,)),
            ],
            compiler_params=pltpu.CompilerParams(
                collective_id=0, vmem_limit_bytes=32 * 1024 * 1024,
                disable_bounds_checks=True, disable_semaphore_checks=True),
        )(xt)
        return o.reshape(m, 1)
    return kern


pallas_dist_mean_ax1_xy_m4096_n1024_kernel = make(shift=7, ahead=14)
```

```python
import jax
import jax.numpy as jnp
from jax import lax
from jax.experimental import pallas as pl
from jax.experimental.pallas import tpu as pltpu

_MESH = pl.DeviceIdType.MESH

_PAIRS = 16
_GROUPS = 16
_TILES = 8
_BLOCK = _GROUPS * _TILES
_ROUNDS = 2 * _GROUPS


def _tree_sum(vs):
    vs = list(vs)
    while len(vs) > 1:
        vs = [vs[i] + vs[i + 1] if i + 1 < len(vs) else vs[i] for i in range(0, len(vs), 2)]
    return vs[0]


def make(_SHIFT=7, _LEAD=28, _TAIL=8, _TAIL_Q1=4, _FILL=4, _FINAL=4, _AHEAD=3, vmem_out=True, order=None):
    last = _PAIRS - 1
    short = _ROUNDS - _TAIL
    regular = min(short, _ROUNDS - pl.cdiv(_LEAD, 8))

    filler = [_SHIFT + i for i in range(_FILL * _TILES)]
    groups = sorted({t // _TILES for t in filler}, key=lambda g: -sum(t // _TILES == g for t in filler))
    final = sorted(groups[:_FINAL])
    stage2 = [max(t for t in filler if t // _TILES == g) for g in final]
    stage1 = [t for t in filler if t // _TILES in final and t not in stage2]
    pieces = [g * _TILES + _SHIFT for g in range(_TAIL - 1, _FILL - 1, -1)]
    stage0 = [t + j for t in pieces for j in range(_TILES)]
    stage0 += [t for t in filler if t // _TILES not in final]
    tail_tiles = stage0 + stage1 + stage2
    stages = (
        (0, len(stage0)),
        (len(stage0), len(stage1)),
        (len(stage0) + len(stage1), len(stage2)),
    )

    queues = [
        [(p, t) for t in range(_ROUNDS) for p in range(1 - q, _PAIRS, 2) if p != last or t < short]
        for q in range(2)
    ]
    for i in range(len(pieces)):
        queues[1 if i < _TAIL_Q1 else 0].append((None, i * _TILES, _TILES))
    queues[1] += [(None, i, 1) for i in range(len(pieces) * _TILES, len(tail_tiles))]

    def body(x_ref, o_ref, buf, head, part, recv, round_sem, tail_sem, send_sem, recv_sem, *, scale):
        def staged(t, tile, n):
            return buf.at[pl.ds(t * _BLOCK + tile, n)]

        def read(tile, dst, sem, queue):
            src = x_ref.at[pl.ds(tile, dst.shape[0])]
            pltpu.make_async_copy(src, dst, sem).start(priority=queue)

        def wait(filled, sem):
            pltpu.make_async_copy(filled, filled, sem).wait()

        def read_boundary(p, half, queue):
            tile = (2 * p + half + 1) * _BLOCK - _TILES + _SHIFT
            if _SHIFT and (p, half) == (last, 1):
                rest = _TILES - _SHIFT
                read(tile, staged(half, p * _TILES, rest), round_sem.at[half], queue)
                read(0, staged(half, p * _TILES + rest, _SHIFT), round_sem.at[half], queue)
            else:
                read(tile, staged(half, p * _TILES, _TILES), round_sem.at[half], queue)

        for p, t in queues[1][:16]:
            read_boundary(p, t, 1)

        my_x = lax.axis_index("x")
        my_y = lax.axis_index("y")
        peer = (my_x, 1 - my_y)

        def group(t):
            if isinstance(t, int):
                return _GROUPS - t if t <= _GROUPS else _ROUNDS - 1 - t
            return jnp.where(t <= _GROUPS, _GROUPS - t, _ROUNDS - 1 - t)

        def offset(t):
            if isinstance(t, int):
                half = 1 - my_y if t <= _GROUPS else my_y
            else:
                half = jnp.where(t <= _GROUPS, 1 - my_y, my_y)
            return half * _BLOCK + group(t) * _TILES + _SHIFT

        def read_piece(p, t, off, queue):
            read(2 * p * _BLOCK + off, staged(t, p * _TILES, _TILES), round_sem.at[t], queue)

        def read_entry(entry, queue):
            if entry[0] is None:
                _, i, n = entry
                stage = max(s for s in range(3) if i >= stages[s][0])
                tile = (2 * last + my_y) * _BLOCK + tail_tiles[i]
                read(tile, staged(_ROUNDS, i, n), tail_sem.at[stage], queue)
            elif entry[1] < 2:
                read_boundary(*entry, queue)
            else:
                read_piece(*entry, offset(entry[1]), queue)

        def read_entries(lo, hi):
            for i in range(lo, hi):
                if i < len(queues[0]):
                    read_entry(queues[0][i], 0)
                if i + _LEAD < len(queues[1]):
                    read_entry(queues[1][i + _LEAD], 1)

        def read_round(t):
            offs = {d: offset(t + d) for d in sorted({0, _LEAD // 8, (_LEAD + 7) // 8})}
            for k in range(8):
                read_piece(2 * k + 1, t, offs[0], 0)
                d, k1 = divmod(_LEAD + k, 8)
                read_piece(2 * k1, t + d, offs[d], 1)

        for entry in queues[1][16:_LEAD]:
            read_entry(entry, 1)
        read_entries(0, 16)
        pl.loop(2, 2 + _AHEAD)(read_round)

        barrier = pltpu.get_barrier_semaphore()
        pl.semaphore_signal(barrier, inc=1, device_id=peer, device_id_type=_MESH)

        diag = lax.broadcasted_iota(jnp.int32, (8, 128), 1) - lax.broadcasted_iota(jnp.int32, (8, 128), 0)
        zeros = jnp.zeros((8, 128), jnp.float32)

        def place(g, tiles, other):
            sums = jnp.sum(_tree_sum(tiles), axis=1, keepdims=True)
            return jnp.where(diag == g * 8, sums, other)

        def row(acc):
            return jnp.sum(acc, axis=0, keepdims=True)

        def split(t, p):
            v = staged(t, p * _TILES, _TILES)[...]
            tiles = [v[j] for j in range(_TILES)]
            return tiles[: _TILES - _SHIFT], tiles[_TILES - _SHIFT :]

        def add_round(t, accs):
            g = group(t)
            out = []
            for p, acc in enumerate(accs):
                lo, hi = split(t, p)
                new = place(g, lo, zeros)
                out.append(acc + (place(g + 1, hi, new) if hi else new))
            return tuple(out)

        def to_peer(src, dst, i):
            return pltpu.make_async_remote_copy(
                src, dst, send_sem.at[i], recv_sem.at[i], device_id=peer, device_id_type=_MESH
            )

        wait(staged(0, 0, _BLOCK), round_sem.at[0])
        wait(staged(1, 0, _BLOCK), round_sem.at[1])

        for p in range(_PAIRS):
            lo0, hi0 = split(0, p)
            lo1, _ = split(1, p)
            _, hi1 = split(1, (p + last) & last)
            head[0, p] = place(_GROUPS - 1, lo0, place(0, hi1, zeros) if hi1 else zeros)
            head[1, p] = place(_GROUPS - 1, lo1, place(0, hi0, zeros) if hi0 else zeros)

        def their_round(t, accs):
            wait(staged(t, 0, _BLOCK), round_sem.at[t])
            read_round(t + _AHEAD)
            return add_round(t, accs)

        accs = tuple(head[1 - my_y, p] for p in range(_PAIRS))
        accs = lax.fori_loop(2, _GROUPS + 1, their_round, accs)
        for p in range(_PAIRS):
            part[p] = row(accs[p])
        pl.semaphore_wait(barrier, 1)
        partials = to_peer(part, recv, 0)
        partials.start()

        def my_round(t, accs):
            wait(staged(t, 0, _BLOCK), round_sem.at[t])
            pl.when(t + _AHEAD < regular)(lambda: read_round(t + _AHEAD))

            @pl.when(t + _AHEAD == regular)
            def _():
                read_entries(regular * 8, max(len(queues[0]), len(queues[1]) - _LEAD))

            return add_round(t, accs)

        def my_short_round(t, accs):
            wait(staged(t, 0, last * _TILES), round_sem.at[t])
            return add_round(t, accs)

        accs = tuple(head[my_y, p] for p in range(_PAIRS))
        *accs, acc_last = lax.fori_loop(_GROUPS + 1, short, my_round, accs)
        partials.wait()
        accs = lax.fori_loop(short, _ROUNDS - 1, my_short_round, tuple(accs))
        accs = my_short_round(_ROUNDS - 1, accs)

        def rows(p, n, half):
            return o_ref.at[pl.ds(p, n), pl.ds(half, 1)]

        for p in range(last):
            o_ref[p, pl.ds(my_y, 1)] = ((row(accs[p]) + recv[p]) * scale)[None]
        means = to_peer(rows(0, last, my_y), rows(0, last, my_y), 1)
        means.start()

        def stage(s):
            start, n = stages[s]
            if n:
                wait(staged(_ROUNDS, start, n), tail_sem.at[s])
            by_group = {}
            for i in range(start, start + n):
                by_group.setdefault(tail_tiles[i] // _TILES, []).append(buf[_ROUNDS * _BLOCK + i])
            return by_group

        early = stage(0)
        new = zeros
        for g in sorted(early):
            if g not in final:
                new = place(g, early[g], new)
        middle = stage(1)
        sums = {g: early.get(g, []) + middle.get(g, []) for g in final}
        sums = {g: [_tree_sum(v)] if v else [] for g, v in sums.items()}
        late = stage(2)
        done = row(acc_last + new) + recv[last]
        new = zeros
        for g in (order or final):
            new = place(g, sums[g] + late[g], new)
        o_ref[last, pl.ds(my_y, 1)] = ((done + row(new)) * scale)[None]
        closing = to_peer(rows(last, 1, my_y), rows(last, 1, my_y), 2)
        closing.start()

        means.wait_send()
        closing.wait_send()
        to_peer(rows(0, last, 1 - my_y), rows(0, last, 1 - my_y), 1).wait_recv()
        to_peer(rows(last, 1, 1 - my_y), rows(last, 1, 1 - my_y), 2).wait_recv()

    def kernel(x):
        m, n = x.shape
        assert (m, n) == (2 * _PAIRS * _GROUPS * 8, _TILES * 128), x.shape
        tiles = x.reshape(m // 8, 8, _TILES, 128).transpose(0, 2, 1, 3).reshape(-1, 8, 128)
        out = pl.pallas_call(
            lambda *refs: body(*refs, scale=1.0 / (2 * n)),
            out_shape=(pltpu.VMEM if vmem_out else jax.ShapeDtypeStruct)((_PAIRS, 2, 1, 128), jnp.float32),
            in_specs=[pl.BlockSpec(memory_space=pl.ANY)],
            out_specs=pl.BlockSpec(memory_space=pltpu.VMEM),
            scratch_shapes=[
                pltpu.VMEM((_ROUNDS * _BLOCK + len(tail_tiles), 8, 128), jnp.float32),
                pltpu.VMEM((2, _PAIRS, 8, 128), jnp.float32),
                pltpu.VMEM((_PAIRS, 1, 128), jnp.float32),
                pltpu.VMEM((_PAIRS, 1, 128), jnp.float32),
                pltpu.SemaphoreType.DMA((_ROUNDS,)),
                pltpu.SemaphoreType.DMA((3,)),
                pltpu.SemaphoreType.DMA((3,)),
                pltpu.SemaphoreType.DMA((3,)),
            ],
            compiler_params=pltpu.CompilerParams(
                collective_id=0,
                vmem_limit_bytes=32 * 1024 * 1024,
                disable_bounds_checks=True,
                disable_semaphore_checks=True,
            ),
        )(tiles)
        return out.reshape(m, 1)

    return kernel


pallas_dist_mean_ax1_xy_m4096_n1024_kernel = make()
```

```python
import functools

import jax
import jax.numpy as jnp
from jax import lax
from jax.experimental import pallas as pl
from jax.experimental.pallas import tpu as pltpu

_PAIRS = 16
_GROUPS = 16
_TILES = 8
_BLOCK = _GROUPS * _TILES
_ROUNDS = 2 * _GROUPS
_LAST = _PAIRS - 1

_SHIFT = 7
_QUEUE_PAIRS = ((0, 5, 2, 7, 8, 13, 10, 15), (1, 4, 3, 6, 9, 12, 11, 14))
_LEAD = 28
_AHEAD = 3
_CLOSING = 8
_SPLIT = 4


def _group(i):
    return i ^ (i >> 1) ^ (_GROUPS - 1)


_SHORT = _ROUNDS - _CLOSING
_REGULAR = min(_SHORT, _ROUNDS - (_LEAD + 7) // 8)

_starts = [_group(i) * _TILES + _SHIFT for i in range(_GROUPS - _CLOSING, _GROUPS)]
_whole = [t + j for t in _starts[:-_SPLIT] for j in range(_TILES)]
_single = sorted(t + j for t in _starts[-_SPLIT:] for j in range(_TILES))
_FINAL = sorted({t // _TILES for t in _single})[-_SPLIT:]
_ends = [max(t for t in _single if t // _TILES == g) for g in _FINAL]
_STAGES = (
    _whole + [t for t in _single if t // _TILES not in _FINAL],
    [t for t in _single if t // _TILES in _FINAL and t not in _ends],
    _ends,
)
_CLOSING_TILES = [(s, t) for s, stage in enumerate(_STAGES) for t in stage]

_QUEUES = tuple(
    [(p, t) for t in range(_ROUNDS) for p in pairs if p != _LAST or t < _SHORT]
    for pairs in _QUEUE_PAIRS
)
_QUEUES[1].extend((None, i, _TILES) for i in range(0, len(_whole), _TILES))
_QUEUES[1].extend((None, i, 1) for i in range(len(_whole), len(_CLOSING_TILES)))


def _tree_sum(vs):
    vs = list(vs)
    while len(vs) > 1:
        vs = [a + b for a, b in zip(vs[0::2], vs[1::2])] + vs[len(vs) & ~1 :]
    return vs[0]


def _mean_kernel(
    x_ref, o_ref, buf, first, sent, received, round_sem, stage_sem, send_sem, recv_sem,
    *, scale,
):
    def staged(t, tile, n):
        return buf.at[pl.ds(t * _BLOCK + tile, n)]

    def read(tile, dst, sem, queue):
        src = x_ref.at[pl.ds(tile, dst.shape[0])]
        pltpu.make_async_copy(src, dst, sem).start(priority=queue)

    def wait(filled, sem):
        pltpu.make_async_copy(filled, filled, sem).wait()

    def read_boundary(p, half, queue):
        tile = (2 * p + half + 1) * _BLOCK - _TILES + _SHIFT
        if (p, half) == (_LAST, 1):
            rest = _TILES - _SHIFT
            read(tile, staged(half, p * _TILES, rest), round_sem.at[half], queue)
            read(0, staged(half, p * _TILES + rest, _SHIFT), round_sem.at[half], queue)
        else:
            read(tile, staged(half, p * _TILES, _TILES), round_sem.at[half], queue)

    for p, t in _QUEUES[1][:_PAIRS]:
        read_boundary(p, t, 1)

    my_y = lax.axis_index("y")
    neighbour = (lax.axis_index("x"), 1 - my_y)

    def pick(theirs, a, b):
        return (a if theirs else b) if isinstance(theirs, bool) else jnp.where(theirs, a, b)

    def group(t):
        return _group(pick(t <= _GROUPS, t - 1, t - _GROUPS))

    def offset(t):
        half = pick(t <= _GROUPS, 1 - my_y, my_y)
        return half * _BLOCK + group(t) * _TILES + _SHIFT

    def read_piece(p, t, start, queue):
        dst = staged(t, p * _TILES, _TILES)
        read(2 * p * _BLOCK + start, dst, round_sem.at[t], queue)

    def read_entry(entry, queue):
        if entry[0] is None:
            _, i, n = entry
            stage, tile = _CLOSING_TILES[i]
            tile = (2 * _LAST + my_y) * _BLOCK + tile
            read(tile, staged(_ROUNDS, i, n), stage_sem.at[stage], queue)
        elif entry[1] < 2:
            read_boundary(*entry, queue)
        else:
            read_piece(*entry, offset(entry[1]), queue)

    def read_entries(lo, hi):
        for i in range(lo, hi):
            if i < len(_QUEUES[0]):
                read_entry(_QUEUES[0][i], 0)
            if i + _LEAD < len(_QUEUES[1]):
                read_entry(_QUEUES[1][i + _LEAD], 1)

    def read_round(t):
        starts = {d: offset(t + d) for d in (0, _LEAD // 8, (_LEAD + 7) // 8)}
        for k in range(8):
            read_piece(_QUEUE_PAIRS[0][k], t, starts[0], 0)
            d, k1 = divmod(_LEAD + k, 8)
            read_piece(_QUEUE_PAIRS[1][k1], t + d, starts[d], 1)

    for entry in _QUEUES[1][_PAIRS:_LEAD]:
        read_entry(entry, 1)
    read_entries(0, _PAIRS)
    pl.loop(2, 2 + _AHEAD)(read_round)

    barrier = pltpu.get_barrier_semaphore()
    pl.semaphore_signal(
        barrier, inc=1, device_id=neighbour, device_id_type=pl.DeviceIdType.MESH
    )

    iota = functools.partial(lax.broadcasted_iota, jnp.int32, (8, 128))
    diagonal = iota(1) - iota(0)
    zeros = jnp.zeros((8, 128), jnp.float32)

    def place(g, tiles, other):
        sums = jnp.sum(_tree_sum(tiles), axis=1, keepdims=True)
        return jnp.where(diagonal == g * 8, sums, other)

    def row(acc):
        return jnp.sum(acc, axis=0, keepdims=True)

    def parts(t, p):
        piece = staged(t, p * _TILES, _TILES)[...]
        tiles = [piece[j] for j in range(_TILES)]
        return tiles[: _TILES - _SHIFT], tiles[_TILES - _SHIFT :]

    def add_round(t, accs):
        g = group(t)
        out = []
        for p, acc in enumerate(accs):
            own, following = parts(t, p)
            out.append(acc + place(g + 1, following, place(g, own, zeros)))
        return tuple(out)

    def to_neighbour(src, dst, i):
        return pltpu.make_async_remote_copy(
            src, dst, send_sem.at[i], recv_sem.at[i],
            device_id=neighbour, device_id_type=pl.DeviceIdType.MESH,
        )

    wait(staged(0, 0, _BLOCK), round_sem.at[0])
    wait(staged(1, 0, _BLOCK), round_sem.at[1])
    for p in range(_PAIRS):
        own0, following0 = parts(0, p)
        own1, _ = parts(1, p)
        _, following1 = parts(1, (p - 1) % _PAIRS)
        first[0, p] = place(_GROUPS - 1, own0, place(0, following1, zeros))
        first[1, p] = place(_GROUPS - 1, own1, place(0, following0, zeros))

    def their_round(t, accs):
        wait(staged(t, 0, _BLOCK), round_sem.at[t])
        read_round(t + _AHEAD)
        return add_round(t, accs)

    accs = tuple(first[1 - my_y, p] for p in range(_PAIRS))
    accs = lax.fori_loop(2, _GROUPS + 1, their_round, accs)
    for p in range(_PAIRS):
        sent[p] = row(accs[p])
    pl.semaphore_wait(barrier, 1)
    partials = to_neighbour(sent, received, 0)
    partials.start()

    def my_round(t, accs):
        wait(staged(t, 0, _BLOCK), round_sem.at[t])

        @pl.when(t + _AHEAD < _REGULAR)
        def _():
            read_round(t + _AHEAD)

        @pl.when(t + _AHEAD == _REGULAR)
        def _():
            read_entries(8 * _REGULAR, max(len(_QUEUES[0]), len(_QUEUES[1]) - _LEAD))

        return add_round(t, accs)

    def my_short_round(t, accs):
        wait(staged(t, 0, _LAST * _TILES), round_sem.at[t])
        return add_round(t, accs)

    accs = tuple(first[my_y, p] for p in range(_PAIRS))
    *accs, acc_last = lax.fori_loop(_GROUPS + 1, _SHORT, my_round, accs)
    partials.wait()
    accs = lax.fori_loop(_SHORT, _ROUNDS - 1, my_short_round, tuple(accs))
    accs = my_short_round(_ROUNDS - 1, accs)

    def share(p, n, half, i):
        rows = o_ref.at[pl.ds(p, n), pl.ds(half, 1)]
        return to_neighbour(rows, rows, i)

    for p in range(_LAST):
        o_ref[p, pl.ds(my_y, 1)] = ((row(accs[p]) + received[p]) * scale)[None]
    means = share(0, _LAST, my_y, 1)
    means.start()

    def arrived(s):
        index = [i for i, (stage, _) in enumerate(_CLOSING_TILES) if stage == s]
        wait(staged(_ROUNDS, index[0], len(index)), stage_sem.at[s])
        groups = {}
        for i in index:
            tile = buf[_ROUNDS * _BLOCK + i]
            groups.setdefault(_CLOSING_TILES[i][1] // _TILES, []).append(tile)
        return groups

    early = arrived(0)
    new = zeros
    for g in sorted(early):
        if g not in _FINAL:
            new = place(g, early[g], new)
    middle = arrived(1)
    sums = {g: _tree_sum(early.get(g, []) + middle[g]) for g in _FINAL}
    late = arrived(2)
    done = row(acc_last + new) + received[_LAST]
    new = zeros
    for g in _FINAL:
        new = place(g, [sums[g]] + late[g], new)
    o_ref[_LAST, pl.ds(my_y, 1)] = ((done + row(new)) * scale)[None]
    closing = share(_LAST, 1, my_y, 2)
    closing.start()

    means.wait_send()
    closing.wait_send()
    share(0, _LAST, 1 - my_y, 1).wait_recv()
    share(_LAST, 1, 1 - my_y, 2).wait_recv()


def pallas_dist_mean_ax1_xy_m4096_n1024_kernel(x: jax.Array):
    m, n = x.shape
    assert (m, n) == (2 * _PAIRS * _GROUPS * 8, _TILES * 128), x.shape
    tiles = x.reshape(m // 8, 8, _TILES, 128).transpose(0, 2, 1, 3).reshape(-1, 8, 128)
    out = pl.pallas_call(
        functools.partial(_mean_kernel, scale=1.0 / (2 * n)),
        out_shape=jax.ShapeDtypeStruct((_PAIRS, 2, 1, 128), jnp.float32),
        in_specs=[pl.BlockSpec(memory_space=pl.ANY)],
        out_specs=pl.BlockSpec(memory_space=pltpu.VMEM),
        scratch_shapes=[
            pltpu.VMEM((_ROUNDS * _BLOCK + len(_CLOSING_TILES), 8, 128), jnp.float32),
            pltpu.VMEM((2, _PAIRS, 8, 128), jnp.float32),
            pltpu.VMEM((_PAIRS, 1, 128), jnp.float32),
            pltpu.VMEM((_PAIRS, 1, 128), jnp.float32),
            pltpu.SemaphoreType.DMA((_ROUNDS,)),
            pltpu.SemaphoreType.DMA((len(_STAGES),)),
            pltpu.SemaphoreType.DMA((3,)),
            pltpu.SemaphoreType.DMA((3,)),
        ],
        compiler_params=pltpu.CompilerParams(
            collective_id=0,
            vmem_limit_bytes=32 * 1024 * 1024,
            disable_bounds_checks=True,
            disable_semaphore_checks=True,
        ),
    )(tiles)
    return out.reshape(m, 1)
```
